```python
import numpy as np

kernel_name = "dist_sparse_attn_strided_kvseq_b1_sq256_skv4096_hq8_dh128"

def setup_inputs():
    x = np.random.randn(1, 256, 1024).astype(np.float32)
    Wq = np.random.randn(1024, 1024).astype(np.float32) * 0.02
    K_ext = np.random.randn(1, 16384, 8, 128).astype(np.float32)
    V_ext = np.random.randn(1, 16384, 8, 128).astype(np.float32)
    Wo = np.random.randn(1024, 1024).astype(np.float32) * 0.02
    return {"x": x, "Wq": Wq, "K_ext": K_ext, "V_ext": V_ext, "Wo": Wo}

def reference(x, Wq, K_ext, V_ext, Wo):
    B, Sq, Skv, Hq, Dh = 1, 256, 16384, 8, 128
    Q = (x @ Wq).reshape(B, Sq, Hq, Dh)
    qb = (np.arange(Sq) // 64)[:, None]
    kb = (np.arange(Skv) // 64)[None, :]
    mask = (qb == kb) | ((kb % 4) == (qb % 4))
    scores = np.einsum('bihd,bjhd->bhij', Q, K_ext).astype(np.float32) * 0.08838834764831843
    scores = np.where(mask[None, None, :, :], scores, -1e9)
    scores_max = scores.max(axis=-1, keepdims=True)
    w = np.exp(scores - scores_max)
    row_keep = mask.any(axis=1)
    w_sum = np.where(row_keep[None, None, :, None], w.sum(axis=-1, keepdims=True), 1.0)
    w = w / w_sum
    w = np.where(row_keep[None, None, :, None], w, 0.0)
    ctx = np.einsum('bhij,bjhd->bihd', w, V_ext).reshape(B, Sq, Hq * Dh)
    return ctx @ Wo
```

```python
import contextlib
import functools
import math

import jax
import jax.numpy as jnp
from jax import lax
from jax.experimental import pallas as pl
from jax.experimental.pallas import tpu as pltpu

F32, BF16 = jnp.float32, jnp.bfloat16
N_DEV = 4
BLK = 64
N_CLS = 4
HEADS = 8
DH = 128
DM = HEADS * DH
N_KB = 16
N_KEYS = N_KB * BLK
N_UNITS = N_CLS * HEADS
HALF = DM // 2
Q_SCALE = 0.08838834764831843 * math.log2(math.e)

DEFAULTS = dict(
    ne=5,
    lag=4,
    unfuse=28,
    i0=(16, 16, 17, 16),
    qproj=((7, 11, 16, 20), (7, 12, 20, 28)),
    merge=(33, 37, 41, 49),
    proj=(35, 39, 43, 51),
    fwd=(45, 49, 53, 61),
    mid=((53, 57, 61), (57,), (), (57,)),
    xsend=(1, 2, 3, 4),
    wq_cvt=4,
    q_order=(1, 0, 2),
    wo_cuts=(0, 512, 1024),
    late_chunk=False,
    wo7_rows=8,
    wo7_thr="1",
    vsplit=8,
    vlast_nk=32,
    tail="k31 s29 v29 v31 m3 s30 v30 w7 s31",
    p0_peers=(3, 2, 1),
    scopes=False,
    sem_checks=True,
    out_dtype=BF16,
)

FIELDS = dict(fetch_q=2, fetch_h=3, attn=2, unit=5, attn_q=2, attn_h=3, q_wait=2, job=4, job_arg=3)
JOBS = ("none", "barrier", "send_x", "cast_wq", "project_q", "cast_wo", "send_wo", "merge", "project", "forward", "mid")


def build(**overrides):
    cfg = {**DEFAULTS, **overrides}
    NE = cfg["ne"]
    NM = HEADS - 1 - NE
    FIRST_MID = N_CLS * NE
    FIRST_LAST = N_UNITS - N_CLS
    LAST = N_UNITS - 1
    N_TICKS = 2 * N_UNITS - 2
    CHUNKS = [pl.ds(a, b - a) for a, b in zip(cfg["wo_cuts"], cfg["wo_cuts"][1:])]
    NCH = len(CHUNKS)
    scope = jax.named_scope if cfg["scopes"] else (lambda name: contextlib.nullcontext())

    units = ([(q, h) for q in range(N_CLS) for h in range(NE)]
             + [(q, h) for q in range(N_CLS) for h in range(NE, HEADS - 1)]
             + [(q, HEADS - 1) for q in range(N_CLS)])
    wo_order = list(range(NE, HEADS - 1)) + list(range(NE))

    def schedule(dev):
        jobs = {0: ("barrier", 0)}

        def add(name, ticks, args=range(N_CLS)):
            for t, arg in zip(ticks, args):
                assert t not in jobs, (dev, name, t)
                jobs[t] = (name, arg)

        busy = ()
        if dev == 0:
            add("cast_wo", [t for t in range(1, HEADS + 1) if t != 1 + NM], wo_order)
            add("send_wo", [1 + NM])
            add("merge", cfg["merge"])
            add("project", cfg["proj"])
            busy = cfg["merge"] + cfg["proj"]
        elif dev == 2:
            add("send_x", cfg["xsend"], range(N_CLS - len(cfg["xsend"]), N_CLS))
        else:
            busy = cfg["qproj"][dev >> 1]
            add("cast_wq", [cfg["wq_cvt"]])
            add("project_q", busy)
            add("forward", cfg["fwd"])
        add("mid", cfg["mid"][dev])

        attn, i = {}, cfg["i0"][dev]
        for j in range(N_UNITS):
            if j >= cfg["unfuse"]:
                i = max(i, 2 * j - 1 + cfg["lag"])
                attn[i] = (2, j)
                i += 1
            i = max(i, 2 * j + cfg["lag"])
            while i in busy:
                i += 1
            attn[i] = (3 if 0 < j < cfg["unfuse"] else 1, j)
            i += 1

        words = []
        for i in range(N_TICKS):
            kind, j = attn.get(i, (0, 0))
            q, h = units[j]
            remote_half = kind & 1 and h % (HEADS // 2) == 0 and dev != 1 + 2 * (h // (HEADS // 2))
            job, arg = jobs.get(i, ("none", 0))
            values = dict(fetch_q=units[i >> 1][0], fetch_h=units[i >> 1][1], attn=kind, unit=j, attn_q=q, attn_h=h,
                          q_wait=int(remote_half), job=JOBS.index(job), job_arg=arg)
            word, shift = 0, 0
            for name, bits in FIELDS.items():
                word |= values[name] << shift
                shift += bits
            words.append(word)
        return words

    def body(x_hbm, wq_hbm, k_hbm, v_hbm, wo_hbm, out_ref,
             kbuf, vbuf, x_f32, wq_f32, wo_f32, x_bf, wq_bf, wo_bf, q_bf, p_bf,
             acc_own, acc_in, stat_own, stat_in, ctx, ctx_mid, ctx_last, piece, pre, acc_half, plan,
             k_sem, v_sem, w_sem, wl_sem, x_rsem, wo_rsem, q_rsem, acc_rsem, stat_rsem, piece_rsem,
             acc_ssem, stat_ssem, last_ssem, role_ssem):
        me = lax.axis_index("i")
        is_p0 = me == 0
        is_p2 = me == 2
        is_odd = (me & 1) == 1
        half = me >> 1

        def by_role(a, b, c):
            return jnp.where(is_p0, a, jnp.where(is_odd, b, c))

        def remote(src, dst, ssem, rsem, dev):
            return pltpu.make_async_remote_copy(
                src, dst, ssem, rsem, device_id=(dev,), device_id_type=pl.DeviceIdType.MESH)

        def wait_filled(buf, sem):
            pltpu.make_async_copy(buf, buf, sem).wait()

        def fetch_kv(hbm, buf, sem, u, q, h):
            for k0 in (0, BLK // 2):
                for b in range(N_KB):
                    pltpu.make_async_copy(
                        hbm.at[b, q, pl.ds(k0, BLK // 2), h], buf.at[u, pl.ds(b * BLK + k0, BLK // 2)],
                        sem.at[u]).start(priority=b & 1)

        def fetch_last_v():
            q, h = units[LAST]
            nk = cfg["vlast_nk"]
            for b in range(N_KB):
                for k0 in range(0, BLK, nk):
                    pltpu.make_async_copy(
                        v_hbm.at[b, q, pl.ds(k0, nk), h], vbuf.at[LAST, pl.ds(b * BLK + k0, nk)],
                        v_sem.at[LAST + (b >= cfg["vsplit"])]).start(priority=1)

        def fetch_rows(hbm, buf, row0, n_rows, sem):
            for r in range(0, n_rows, 8):
                rows = pl.ds(pl.multiple_of(row0 + r, 8), 8)
                for c in range(2):
                    cols = pl.ds(c * HALF, HALF)
                    pltpu.make_async_copy(hbm.at[rows, cols], buf.at[rows, cols], sem).start(priority=c)

        def fetch_last_wo():
            for c in range(NCH):
                for n, r in enumerate(range(0, DH, cfg["wo7_rows"])):
                    at = (pl.ds(DM - DH + r, cfg["wo7_rows"]), CHUNKS[c])
                    pltpu.make_async_copy(wo_hbm.at[at], wo_f32.at[at], wl_sem.at[c]).start(
                        priority=int(cfg["wo7_thr"][n % len(cfg["wo7_thr"])]))

        def head_rows(h):
            return pl.ds(pl.multiple_of(h * DH, DH), DH)

        def cls_rows(q):
            return pl.ds(pl.multiple_of(q * BLK, BLK), BLK)

        @pl.when(is_p2)
        def _():
            @pl.loop(0, N_CLS)
            def _(q):
                fetch_rows(x_hbm, x_f32, q * BLK, BLK, w_sem.at[q])

        fetch_kv(k_hbm, kbuf, k_sem, 0, *units[0])

        pa, pb, pc = cfg["p0_peers"]
        peers = (jnp.where(is_p0, pa, 0), by_role(pb, me ^ 2, 1), by_role(pc, 2, 3))
        barrier = pltpu.get_barrier_semaphore()
        for dev in peers:
            pl.semaphore_signal(barrier, inc=1, device_id=(dev,), device_id_type=pl.DeviceIdType.MESH)

        @pl.when(is_p0)
        def _():
            @pl.loop(0, HEADS - 1)
            def _(g):
                h = jnp.where(g < NM, g + NE, g - NM)
                fetch_rows(wo_hbm, wo_f32, h * DH, DH, w_sem.at[h])

        @pl.when(is_odd)
        def _():
            @pl.loop(0, HEADS)
            def _(g):
                for r in range(0, DH, 8):
                    rows = pl.ds(pl.multiple_of(g * DH + r, 8), 8)
                    pltpu.make_async_copy(
                        wq_hbm.at[rows, pl.ds(pl.multiple_of(half * HALF, HALF), HALF)],
                        wq_f32.at[rows], w_sem.at[0]).start(priority=(r // 8) & 1)

        for dev in range(N_DEV):
            @pl.when(me == dev)
            def _():
                for i, word in enumerate(schedule(dev)):
                    plan[i] = word

        row_id = lax.broadcasted_iota(jnp.int32, (BLK, DH), 0)
        lane_id = lax.broadcasted_iota(jnp.int32, (BLK, DH), 1)

        def scores_phase(u, q, h):
            s = lax.dot_general(q_bf[q, h], kbuf[u].astype(BF16), (((1,), (1,)), ((), ())),
                                preferred_element_type=F32)
            m = jnp.max(s, axis=1, keepdims=True)
            p = jnp.exp2(s - m)
            l = jnp.sum(p, axis=1, keepdims=True)
            p_bf[u & 1] = p.astype(BF16)
            diag = (lane_id & (BLK - 1)) == row_id
            stat_own[u, 0:1] = jnp.sum(jnp.where(diag, m, 0.0), axis=0, keepdims=True)
            stat_own[u, 1:2] = jnp.sum(jnp.where(diag, l, 0.0), axis=0, keepdims=True)

        def values_phase(u):
            acc_own[u] = jnp.dot(p_bf[u & 1], vbuf[u].astype(BF16),
                                 preferred_element_type=F32).astype(BF16)

        def share(u, own, landing, ssem, rsem):
            for i, dev in enumerate(peers):
                @pl.when((u >= FIRST_MID) | (jnp.logical_not(is_p0) if i == 0 else False))
                def _():
                    remote(own.at[u], landing.at[u, ((dev - me) & 3) - 1], ssem.at[i], rsem.at[u], dev).start()

        def scores_step(u, q, h):
            with scope("kwait"):
                wait_filled(kbuf.at[u], k_sem.at[u])
            with scope("s"):
                scores_phase(u, q, h)
            share(u, stat_own, stat_in, stat_ssem, stat_rsem)

        def values_step(u):
            with scope("vwait"):
                wait_filled(vbuf.at[u], v_sem.at[u])
            with scope("v"):
                values_phase(u)
            share(u, acc_own, acc_in, acc_ssem, acc_rsem)

        def merge_weights(u):
            ms = [stat_own[u, 0:1]] + [stat_in[u, i, 0:1] for i in range(N_DEV - 1)]
            ls = [stat_own[u, 1:2]] + [stat_in[u, i, 1:2] for i in range(N_DEV - 1)]
            top = functools.reduce(jnp.maximum, ms)
            scales = [jnp.exp2(m - top) for m in ms]
            inv = 1.0 / sum(a * l for a, l in zip(scales, ls))
            diag = lane_id == row_id
            return [jnp.sum(jnp.where(diag, a * inv, 0.0), axis=1, keepdims=True) for a in scales]

        def weighted_sum(u, w):
            parts = [acc_own[u]] + [acc_in[u, i] for i in range(N_DEV - 1)]
            return sum(wi * a.astype(F32) for wi, a in zip(w, parts)).astype(BF16)

        def merge(u0, n, axis):
            with scope("mwait"):
                for i in range(n):
                    wait_filled(stat_in.at[u0 + i], stat_rsem.at[u0 + i])
                    wait_filled(acc_in.at[u0 + i], acc_rsem.at[u0 + i])
            return jnp.concatenate([weighted_sum(u0 + i, merge_weights(u0 + i)) for i in range(n)], axis=axis)

        mid_rows = wo_bf.at[pl.ds(NE * DH, NM * DH)]

        def job_barrier(_):
            pl.semaphore_wait(barrier, N_DEV - 1)

        def job_send_x(q):
            wait_filled(x_f32.at[cls_rows(q)], w_sem.at[q])
            x_bf[q] = x_f32[cls_rows(q)].astype(BF16)
            for s, dev in enumerate((1, 3)):
                remote(x_bf.at[q], x_bf.at[q], role_ssem.at[s], x_rsem.at[q], dev).start()

        def job_cast_wq(_):
            wait_filled(wq_f32, w_sem.at[0])

            @pl.loop(0, HEADS)
            def _(g):
                wq_bf[head_rows(g)] = wq_f32[head_rows(g)].astype(BF16)

        def job_project_q(q):
            with scope("xwait"):
                wait_filled(x_bf.at[q], x_rsem.at[q])
            qv = jnp.dot(x_bf[q], wq_bf[...], preferred_element_type=F32) * Q_SCALE
            for g in range(HEADS // 2):
                q_bf[q, half * (HEADS // 2) + g] = qv[:, g * DH:(g + 1) * DH].astype(BF16)
            mine = q_bf.at[q, pl.ds(half * (HEADS // 2), HEADS // 2)]
            for s in cfg["q_order"]:
                remote(mine, mine, role_ssem.at[s], q_rsem.at[half * N_CLS + q], peers[s]).start()

        def job_cast_wo(h):
            wait_filled(wo_f32.at[head_rows(h)], w_sem.at[h])
            wo_bf[head_rows(h)] = wo_f32[head_rows(h)].astype(BF16)

        def job_send_wo(_):
            for s, dev in enumerate((1, 3)):
                remote(mid_rows, mid_rows, role_ssem.at[2 + s], wo_rsem, dev).start()

        def job_merge(q):
            ctx[...] = merge(NE * q, NE, axis=1)

        def job_project(q):
            for c in range(2):
                piece[c, cls_rows(q)] = jnp.dot(
                    ctx[...], wo_bf[0:NE * DH, c * HALF:(c + 1) * HALF],
                    preferred_element_type=F32).astype(BF16)
            for first in range(2):
                for s, dev in enumerate((1, 3)):
                    c = s ^ first
                    buf = piece.at[c, cls_rows(q)]
                    remote(buf, buf, role_ssem.at[s], piece_rsem.at[c * N_CLS + q], dev).start()

        def job_forward(q):
            buf = piece.at[half, cls_rows(q)]
            sem = piece_rsem.at[half * N_CLS + q]
            wait_filled(buf, sem)
            remote(buf, buf, role_ssem.at[3], sem, 2).start()

        def job_mid(q):
            with scope("pwait"):
                pl.when((q == 0) & is_odd)(lambda: wait_filled(mid_rows, wo_rsem))
                for c in range(2):
                    @pl.when(is_odd & (half != c))
                    def _():
                        wait_filled(piece.at[c, cls_rows(q)], piece_rsem.at[c * N_CLS + q])
            lhs = merge(FIRST_MID + NM * q, NM, axis=1)
            for c in range(2):
                cols = slice(c * HALF, (c + 1) * HALF)
                pre[cls_rows(q), cols] = piece[c, cls_rows(q)].astype(F32) + jnp.dot(
                    lhs, wo_bf[NE * DH:DM - DH, cols], preferred_element_type=F32)

        jobs = (None, job_barrier, job_send_x, job_cast_wq, job_project_q, job_cast_wo, job_send_wo,
                job_merge, job_project, job_forward, job_mid)

        with scope("barrier"):
            job_barrier(0)
        if len(cfg["xsend"]) < N_CLS:
            with scope("send_x"):
                pl.when(is_p2)(lambda: job_send_x(0))

        @pl.loop(1, N_TICKS)
        def _(i):
            word, shift, f = plan[i], 0, {}
            for name, bits in FIELDS.items():
                f[name] = (word >> shift) & ((1 << bits) - 1)
                shift += bits

            with scope("issue"):
                for parity, (hbm, buf, sem) in enumerate(((k_hbm, kbuf, k_sem), (v_hbm, vbuf, v_sem))):
                    pl.when((i & 1) == parity)(
                        functools.partial(fetch_kv, hbm, buf, sem, i >> 1, f["fetch_q"], f["fetch_h"]))

            u, q, h = f["unit"], f["attn_q"], f["attn_h"]

            @pl.when(f["q_wait"] != 0)
            def _():
                with scope("qwait"):
                    wait_filled(q_bf.at[q, pl.ds(h, HEADS // 2)], q_rsem.at[h + q])

            pl.when(f["attn"] == 1)(lambda: scores_step(u, q, h))
            pl.when(f["attn"] == 2)(lambda: values_step(u - 1))

            @pl.when(f["attn"] == 3)
            def _():
                with scope("kwait"):
                    wait_filled(kbuf.at[u], k_sem.at[u])
                    wait_filled(vbuf.at[u - 1], v_sem.at[u - 1])
                with scope("attn"):
                    values_phase(u - 1)
                    scores_phase(u, q, h)
                share(u - 1, acc_own, acc_in, acc_ssem, acc_rsem)
                share(u, stat_own, stat_in, stat_ssem, stat_rsem)

            @pl.when(f["job"] != 0)
            def _():
                for code in range(1, len(jobs)):
                    @pl.when(f["job"] == code)
                    def _():
                        with scope(JOBS[code]):
                            jobs[code](f["job_arg"])

        n_merged = 0
        for step in cfg["tail"].split():
            kind, arg = step[0], int(step[1:])
            if step == "k31":
                with scope("issue"):
                    fetch_kv(k_hbm, kbuf, k_sem, LAST, *units[LAST])
            elif step == "v31":
                with scope("issue"):
                    fetch_last_v()
            elif kind == "s":
                scores_step(arg, *units[arg])
            elif kind == "v":
                values_step(arg)
            elif kind == "m":
                with scope("mid"):
                    pl.when(is_p0)(functools.partial(job_mid, arg))
            elif kind == "g":
                n_merged = arg
                with scope("merge7a"):
                    @pl.when(is_p0)
                    def _():
                        ctx_last[0:arg * BLK] = merge(FIRST_LAST, arg, axis=0)
            elif kind == "w":
                pl.when(is_p0)(fetch_last_wo)

        split = cfg["vsplit"] * BLK
        for part, keys in enumerate((pl.ds(0, split), pl.ds(split, N_KEYS - split))):
            with scope("vlast_wait"):
                wait_filled(vbuf.at[LAST, keys], v_sem.at[LAST + part])
            with scope("vlast"):
                acc = jnp.dot(p_bf[LAST & 1, :, keys], vbuf[LAST, keys].astype(BF16), preferred_element_type=F32)
                if part == 0:
                    acc_half[...] = acc
                else:
                    acc_own[LAST] = (acc_half[...] + acc).astype(BF16)
                    share(LAST, acc_own, acc_in, last_ssem, acc_rsem)

        @pl.when(jnp.logical_not(is_p0))
        def _():
            @pl.when(is_p2)
            def _():
                pl.loop(NE, HEADS - 1)(lambda h: fetch_rows(wo_hbm, wo_f32, h * DH, DH, w_sem.at[h]))

            fetch_last_wo()

            @pl.when(is_p2)
            def _():
                with scope("mid"):
                    @pl.loop(0, N_CLS)
                    def _(q):
                        ctx_mid[cls_rows(q)] = merge(FIRST_MID + NM * q, NM, axis=1)
                        for c in range(2):
                            wait_filled(piece.at[c, cls_rows(q)], piece_rsem.at[c * N_CLS + q])

                with scope("wo_tail"):
                    pl.loop(NE, HEADS - 1)(job_cast_wo)
                    for c in range(2):
                        cols = slice(c * HALF, (c + 1) * HALF)
                        pre[:, cols] = piece[c].astype(F32) + jnp.dot(
                            ctx_mid[...], wo_bf[NE * DH:DM - DH, cols], preferred_element_type=F32)

            @pl.when(is_odd)
            def _():
                with scope("mid"):
                    pl.loop(len(cfg["mid"][1]), N_CLS, unroll=False)(job_mid)

            if n_merged:
                ctx_last[0:n_merged * BLK] = merge(FIRST_LAST, n_merged, axis=0)

        top = (N_CLS - 1) * BLK
        with scope("merge7"):
            ctx_last[n_merged * BLK:] = merge(FIRST_LAST + n_merged, N_CLS - 1 - n_merged, axis=0)

        def finish_top(cols):
            w = wo_f32[DM - DH:, cols].astype(BF16)
            wo_bf[DM - DH:, cols] = w
            out_ref[0, 0:top, cols] = (pre[0:top, cols] + jnp.dot(
                ctx_last[...], w, preferred_element_type=F32)).astype(out_ref.dtype)

        n_now = NCH - cfg["late_chunk"]
        for c in range(n_now):
            with scope("wo7_wait"):
                wait_filled(wo_f32.at[pl.ds(DM - DH, DH), CHUNKS[c]], wl_sem.at[c])
                if c == n_now - 1:
                    wait_filled(stat_in.at[LAST], stat_rsem.at[LAST])
            with scope("final_a"):
                finish_top(CHUNKS[c])
                if c == n_now - 1:
                    w_last = merge_weights(LAST)

        def drain(buf, ssem):
            remote(buf, buf, ssem, acc_rsem.at[0], me).wait_send()

        @pl.when(is_p0)
        def _():
            drain(acc_own.at[FIRST_MID:LAST], acc_ssem.at[0])
            drain(stat_own.at[FIRST_MID:], stat_ssem.at[0])
            for s in range(2):
                drain(piece, role_ssem.at[s])
                drain(mid_rows, role_ssem.at[2 + s])

        @pl.when(jnp.logical_not(is_p0))
        def _():
            drain(acc_own.at[:LAST], acc_ssem.at[0])
            drain(stat_own, stat_ssem.at[0])

        for s in range(1, N_DEV - 1):
            drain(acc_own.at[FIRST_MID:LAST], acc_ssem.at[s])
            drain(stat_own.at[FIRST_MID:], stat_ssem.at[s])

        @pl.when(is_p2)
        def _():
            for s in range(2):
                drain(x_bf, role_ssem.at[s])

        @pl.when(is_odd)
        def _():
            for s in range(N_DEV - 1):
                drain(q_bf.at[:, pl.ds(half * (HEADS // 2), HEADS // 2)], role_ssem.at[s])
            drain(piece.at[half], role_ssem.at[3])

        with scope("last_wait"):
            if cfg["late_chunk"]:
                wait_filled(wo_f32.at[pl.ds(DM - DH, DH), CHUNKS[-1]], wl_sem.at[NCH - 1])
            wait_filled(acc_in.at[LAST], acc_rsem.at[LAST])
        with scope("final_b"):
            if cfg["late_chunk"]:
                finish_top(CHUNKS[-1])
            out_ref[0, top:] = (pre[top:] + jnp.dot(
                weighted_sum(LAST, w_last), wo_bf[DM - DH:],
                preferred_element_type=F32)).astype(out_ref.dtype)
        for s in range(N_DEV - 1):
            drain(acc_own.at[LAST], last_ssem.at[s])

    def kernel(x, Wq, K_ext, V_ext, Wo):
        sq = x.shape[1]
        kv_shape = (N_KB, N_CLS, BLK, HEADS, DH)
        dma = pltpu.SemaphoreType.DMA
        return pl.pallas_call(
            body,
            out_shape=jax.ShapeDtypeStruct((1, sq, DM), cfg["out_dtype"]),
            in_specs=[pl.BlockSpec(memory_space=pltpu.HBM)] * 5,
            out_specs=pl.BlockSpec(memory_space=pltpu.VMEM),
            scratch_shapes=[
                pltpu.VMEM((N_UNITS, N_KEYS, DH), F32),
                pltpu.VMEM((N_UNITS, N_KEYS, DH), F32),
                pltpu.VMEM((sq, DM), F32),
                pltpu.VMEM((DM, HALF), F32),
                pltpu.VMEM((DM, DM), F32),
                pltpu.VMEM((N_CLS, BLK, DM), BF16),
                pltpu.VMEM((DM, HALF), BF16),
                pltpu.VMEM((DM, DM), BF16),
                pltpu.VMEM((N_CLS, HEADS, BLK, DH), BF16),
                pltpu.VMEM((2, BLK, N_KEYS), BF16),
                pltpu.VMEM((N_UNITS, BLK, DH), BF16),
                pltpu.VMEM((N_UNITS, N_DEV - 1, BLK, DH), BF16),
                pltpu.VMEM((N_UNITS, 2, DH), F32),
                pltpu.VMEM((N_UNITS, N_DEV - 1, 2, DH), F32),
                pltpu.VMEM((BLK, NE * DH), BF16),
                pltpu.VMEM((sq, NM * DH), BF16),
                pltpu.VMEM((sq - BLK, DH), BF16),
                pltpu.VMEM((2, sq, HALF), BF16),
                pltpu.VMEM((sq, DM), F32),
                pltpu.VMEM((BLK, DH), F32),
                pltpu.SMEM((N_TICKS,), jnp.int32),
                dma((N_UNITS,)), dma((N_UNITS + 1,)), dma((HEADS,)), dma((NCH,)),
                dma((N_CLS,)), dma(()), dma((2 * N_CLS,)),
                dma((N_UNITS,)), dma((N_UNITS,)), dma((2 * N_CLS,)),
                dma((N_DEV - 1,)), dma((N_DEV - 1,)), dma((N_DEV - 1,)), dma((N_DEV,)),
            ],
            compiler_params=pltpu.CompilerParams(
                collective_id=0,
                vmem_limit_bytes=64 * 1024 * 1024,
                disable_bounds_checks=not cfg["sem_checks"],
                disable_semaphore_checks=not cfg["sem_checks"],
            ),
        )(x.reshape(sq, DM), Wq, K_ext.reshape(kv_shape), V_ext.reshape(kv_shape), Wo)

    return kernel


def pallas_dist_sparse_attn_strided_kvseq_b1_sq256_skv4096_hq8_dh128_kernel(x, Wq, K_ext, V_ext, Wo):
    return build(sem_checks=False)(x, Wq, K_ext, V_ext, Wo)
```

```python
import functools
import math

import jax
import jax.numpy as jnp
from jax import lax
from jax.experimental import pallas as pl
from jax.experimental.pallas import tpu as pltpu

F32, BF16 = jnp.float32, jnp.bfloat16

N_DEV = 4
BLK = 64
N_QB = 4
HEADS = 8
DH = 128
SQ = N_QB * BLK
DM = HEADS * DH
HALF = DM // 2
N_KB = 16
N_KEYS = N_KB * BLK
Q_SCALE = 0.08838834764831843 * math.log2(math.e)

N_EARLY = 5
N_MID = HEADS - 1 - N_EARLY
UNITS = (
    [(q, h) for q in range(N_QB) for h in range(N_EARLY)]
    + [(q, h) for q in range(N_QB) for h in range(N_EARLY, HEADS - 1)]
    + [(q, HEADS - 1) for q in range(N_QB)]
)
N_UNITS = len(UNITS)
FIRST_MID = N_QB * N_EARLY
FIRST_OF_LAST_HEAD = N_UNITS - N_QB
LAST = N_UNITS - 1

COARSE = (32, (0, 8, 1, 9, 2, 10, 3, 11, 4, 12, 5, 13, 6, 14, 7, 15))
FINE = (16, (0, 8, 2, 10, 1, 9, 3, 11, 4, 12, 6, 14, 5, 13, 7, 15))

N_TICKS = 2 * LAST
FINE_TICKS = 16
FETCH_LEAD = 4
FIRST_ATTN_TICK = (16, 16, 17, 16)
FIRST_SPLIT_UNIT = 28
SCORES, VALUES, BOTH = 1, 2, 3
JOBS = ("send_x", "cast_wq", "project_q", "cast_wo", "send_wo", "merge_early",
        "project_early", "forward", "add_mid")
JOB_TICKS = (
    dict(cast_wo={1: 5, 2: 6, 4: 0, 5: 1, 6: 2, 7: 3, 8: 4}, send_wo={3: 0},
         merge_early={31: 0, 37: 1, 41: 2, 47: 3}, project_early={33: 0, 39: 1, 43: 2, 49: 3},
         add_mid={51: 0, 55: 1, 59: 2}),
    dict(cast_wq={4: 0}, project_q={7: 0, 11: 1, 16: 2, 21: 3},
         forward={43: 0, 47: 1, 52: 2, 57: 3}, add_mid={59: 0}),
    dict(send_x={1: 1, 2: 2, 3: 3}),
    dict(cast_wq={4: 0}, project_q={7: 0, 12: 1, 19: 2, 27: 3},
         forward={43: 0, 47: 1, 52: 2, 57: 3}, add_mid={59: 0}),
)
PLAN_FIELDS = (("fetch_q", 2), ("fetch_h", 3), ("step", 2), ("unit", 5), ("q", 2), ("h", 3),
               ("wait_q", 1), ("job", 4), ("job_arg", 3))


def _plan(dev):
    jobs = {tick: (JOBS.index(name) + 1, arg)
            for name, ticks in JOB_TICKS[dev].items() for tick, arg in ticks.items()}
    steps, tick = {}, FIRST_ATTN_TICK[dev]
    for u in range(N_UNITS):
        if u >= FIRST_SPLIT_UNIT:
            tick = max(tick, 2 * u - 1 + FETCH_LEAD)
            steps[tick] = (VALUES, u)
            tick += 1
        tick = max(tick, 2 * u + FETCH_LEAD)
        while tick in JOB_TICKS[dev].get("project_q", ()):
            tick += 1
        steps[tick] = (BOTH if 0 < u < FIRST_SPLIT_UNIT else SCORES, u)
        tick += 1
    assert steps[N_TICKS] == (SCORES, LAST - 2)

    words = []
    for tick in range(N_TICKS):
        step, u = steps.get(tick, (0, 0))
        q, h = UNITS[u]
        q_half, first_use = h // (HEADS // 2), h % (HEADS // 2) == 0
        values = (*UNITS[tick // 2], step, u, q, h,
                  int(step in (SCORES, BOTH) and first_use and dev != 1 + 2 * q_half),
                  *jobs.get(tick, (0, 0)))
        word, shift = 0, 0
        for (_, bits), value in zip(PLAN_FIELDS, values, strict=True):
            word |= value << shift
            shift += bits
        words.append(word)
    return words


def _aligned(index, size):
    start = index * size
    return pl.ds(start if isinstance(start, int) else pl.multiple_of(start, size), size)


def _remote(src, dst, send_sem, recv_sem, dev):
    return pltpu.make_async_remote_copy(
        src, dst, send_sem, recv_sem, device_id=(dev,), device_id_type=pl.DeviceIdType.MESH)


def _wait_filled(buf, sem):
    pltpu.make_async_copy(buf, buf, sem).wait()


def _dot(a, b):
    return jnp.dot(a, b, preferred_element_type=F32)


def _body(x_hbm, wq_hbm, k_hbm, v_hbm, wo_hbm, out_ref,
          k_buf, v_buf, x_f32, wq_f32, wo_f32, x_bf, wq_bf, wo_bf, q_bf, p_bf,
          acc_own, acc_in, stat_own, stat_in, ctx_early, ctx_mid, out_early, out_acc,
          acc_half, last_terms, plan,
          k_sem, v_sem, w_sem, wo_last_sem,
          x_recv, wo_recv, q_recv, acc_recv, stat_recv, early_recv,
          acc_send, stat_send, last_send, job_send):
    me = lax.axis_index("i")
    is_0, is_2, is_odd = me == 0, me == 2, (me & 1) == 1
    half = me >> 1
    halves = [pl.ds(c * HALF, HALF) for c in range(2)]
    k_refs, v_refs = (k_hbm, k_buf, k_sem), (v_hbm, v_buf, v_sem)
    wo_mid = wo_bf.at[pl.ds(N_EARLY * DH, N_MID * DH)]
    last_head = pl.ds(DM - DH, DH)

    def fetch_unit(refs, u, q, h, pattern=COARSE):
        hbm, buf, sem = refs
        n, order = pattern
        for k0 in range(0, BLK, n):
            for b in order:
                pltpu.make_async_copy(
                    hbm.at[b, q, pl.ds(k0, n), h], buf.at[u, pl.ds(b * BLK + k0, n)],
                    sem.at[u]).start(priority=b & 1)

    def fetch_128_rows(hbm, buf, g):
        for r in range(8):
            for thread in range(2):
                rows = _aligned(16 * g + r + 8 * thread, 8)
                for cols in halves:
                    pltpu.make_async_copy(
                        hbm.at[rows, cols], buf.at[rows, cols], w_sem.at[g]).start(priority=thread)

    def fetch_wo_last_head():
        for c, cols in enumerate(halves):
            for r in range(DM - DH, DM, 16):
                pltpu.make_async_copy(
                    wo_hbm.at[pl.ds(r, 16), cols], wo_f32.at[pl.ds(r, 16), cols],
                    wo_last_sem.at[c]).start(priority=1)

    @pl.when(is_2)
    def _():
        pl.loop(0, SQ // DH)(functools.partial(fetch_128_rows, x_hbm, x_f32))

    fetch_unit(k_refs, 0, *UNITS[0])

    peers = (jnp.where(is_0, 2, 0),
             jnp.where(is_odd, me ^ 2, jnp.where(is_0, 3, 1)),
             jnp.where(is_odd, 2, jnp.where(is_0, 1, 3)))
    barrier = pltpu.get_barrier_semaphore()
    for dev in peers:
        pl.semaphore_signal(barrier, inc=1, device_id=(dev,), device_id_type=pl.DeviceIdType.MESH)

    @pl.when(is_0)
    def _():
        @pl.loop(0, HEADS - 1)
        def _(g):
            fetch_128_rows(wo_hbm, wo_f32, jnp.where(g < N_MID, g + N_EARLY, g - N_MID))

    @pl.when(is_odd)
    def _():
        @pl.loop(0, 8)
        def _(g):
            for r in range(4):
                for n in range(4):
                    rows = _aligned(64 * (g >> 2) + 4 * (g & 3) + r + 16 * n, 8)
                    pltpu.make_async_copy(
                        wq_hbm.at[rows, _aligned(half, HALF)], wq_f32.at[rows],
                        w_sem.at[0]).start(priority=n >> 1)

    for dev in range(N_DEV):
        @pl.when(me == dev)
        def _():
            for tick, word in enumerate(_plan(dev)):
                plan[tick] = word

    row_id = lax.broadcasted_iota(jnp.int32, (BLK, DH), 0)
    lane_id = lax.broadcasted_iota(jnp.int32, (BLK, DH), 1)

    def softmax_numerators(u, q, h):
        s = lax.dot_general(q_bf[q, h], k_buf[u].astype(BF16), (((1,), (1,)), ((), ())),
                            preferred_element_type=F32)
        row_max = jnp.max(s, axis=1, keepdims=True)
        p = jnp.exp2(s - row_max)
        p_bf[u & 1] = p.astype(BF16)
        diag = (lane_id & (BLK - 1)) == row_id
        for i, stat in enumerate((row_max, jnp.sum(p, axis=1, keepdims=True))):
            stat_own[u, i:i + 1] = jnp.sum(jnp.where(diag, stat, 0.0), axis=0, keepdims=True)

    def weighted_values(u):
        acc_own[u] = _dot(p_bf[u & 1], v_buf[u].astype(BF16)).astype(BF16)

    def share(u, own, landing, send, recv):
        for i, dev in enumerate(peers):
            @pl.when((u >= FIRST_MID) | (jnp.logical_not(is_0) if i == 0 else False))
            def _():
                _remote(own.at[u], landing.at[u, ((dev - me) & 3) - 1],
                        send.at[i], recv.at[u], dev).start()

    def scores_step(u, q, h):
        _wait_filled(k_buf.at[u], k_sem.at[u])
        softmax_numerators(u, q, h)
        share(u, stat_own, stat_in, stat_send, stat_recv)

    def values_step(u):
        _wait_filled(v_buf.at[u], v_sem.at[u])
        weighted_values(u)
        share(u, acc_own, acc_in, acc_send, acc_recv)

    def merge_weights(u):
        maxes, sums = (
            [stat_own[u, i:i + 1]] + [stat_in[u, c, i:i + 1] for c in range(N_DEV - 1)]
            for i in range(2))
        top = functools.reduce(jnp.maximum, maxes)
        scales = [jnp.exp2(m - top) for m in maxes]
        inv = 1.0 / sum(a * s for a, s in zip(scales, sums))
        return [jnp.sum(jnp.where(lane_id == row_id, a * inv, 0.0), axis=1, keepdims=True)
                for a in scales]

    def merge(first, count, axis):
        for i in range(count):
            _wait_filled(stat_in.at[first + i], stat_recv.at[first + i])
            _wait_filled(acc_in.at[first + i], acc_recv.at[first + i])
        merged = []
        for i in range(count):
            u = first + i
            parts = [acc_own[u]] + [acc_in[u, c] for c in range(N_DEV - 1)]
            merged.append(
                sum(w * a.astype(F32) for w, a in zip(merge_weights(u), parts)).astype(BF16))
        return jnp.concatenate(merged, axis=axis)

    def wait_early(c, q):
        _wait_filled(out_early.at[c, _aligned(q, BLK)], early_recv.at[c * N_QB + q])

    def send_x(q):
        @pl.when((q & 1) == 0)
        def _():
            _wait_filled(x_f32.at[_aligned(q >> 1, DH)], w_sem.at[q >> 1])

        x_bf[q] = x_f32[_aligned(q, BLK)].astype(BF16)
        for i, dev in enumerate((1, 3)):
            _remote(x_bf.at[q], x_bf.at[q], job_send.at[i], x_recv.at[q], dev).start()

    def cast_wq(_):
        _wait_filled(wq_f32, w_sem.at[0])

        @pl.loop(0, HEADS)
        def _(g):
            wq_bf[_aligned(g, DH)] = wq_f32[_aligned(g, DH)].astype(BF16)

    def project_q(q):
        _wait_filled(x_bf.at[q], x_recv.at[q])
        q_half = _dot(x_bf[q], wq_bf[...]) * Q_SCALE
        for g in range(HEADS // 2):
            q_bf[q, half * (HEADS // 2) + g] = q_half[:, g * DH:(g + 1) * DH].astype(BF16)
        mine = q_bf.at[q, _aligned(half, HEADS // 2)]
        for i, dev in enumerate(peers):
            _remote(mine, mine, job_send.at[i], q_recv.at[half * N_QB + q], dev).start()

    def cast_wo(h):
        _wait_filled(wo_f32.at[_aligned(h, DH)], w_sem.at[h])
        wo_bf[_aligned(h, DH)] = wo_f32[_aligned(h, DH)].astype(BF16)

    def send_wo(_):
        for i, dev in enumerate((1, 3)):
            _remote(wo_mid, wo_mid, job_send.at[2 + i], wo_recv.at[0], dev).start()

    def merge_early(q):
        ctx_early[...] = merge(N_EARLY * q, N_EARLY, axis=1)

    def project_early(q):
        for c, cols in enumerate(halves):
            out_early[c, _aligned(q, BLK)] = _dot(
                ctx_early[...], wo_bf[0:N_EARLY * DH, cols]).astype(BF16)
        for second in range(2):
            for i, dev in enumerate((1, 3)):
                c = i ^ second
                rows = out_early.at[c, _aligned(q, BLK)]
                _remote(rows, rows, job_send.at[i], early_recv.at[c * N_QB + q], dev).start()

    def forward(q):
        wait_early(half, q)
        rows = out_early.at[half, _aligned(q, BLK)]
        _remote(rows, rows, job_send.at[3], early_recv.at[half * N_QB + q], 2).start()

    def add_mid(q):
        pl.when(is_odd & (q == 0))(lambda: _wait_filled(wo_mid, wo_recv.at[0]))
        pl.when(is_odd)(lambda: wait_early(1 - half, q))
        ctx = merge(FIRST_MID + N_MID * q, N_MID, axis=1)
        for c, cols in enumerate(halves):
            out_acc[_aligned(q, BLK), cols] = (
                out_early[c, _aligned(q, BLK)].astype(F32)
                + _dot(ctx, wo_bf[N_EARLY * DH:DM - DH, cols]))

    jobs = (send_x, cast_wq, project_q, cast_wo, send_wo, merge_early,
            project_early, forward, add_mid)

    pl.semaphore_wait(barrier, N_DEV - 1)
    pl.when(is_2)(lambda: send_x(0))

    @pl.loop(1, N_TICKS)
    def _(tick):
        word, shift, f = plan[tick], 0, {}
        for name, bits in PLAN_FIELDS:
            f[name] = (word >> shift) & ((1 << bits) - 1)
            shift += bits

        for parity, refs in enumerate((k_refs, v_refs)):
            for pattern, applies in ((COARSE, tick >= FINE_TICKS), (FINE, tick < FINE_TICKS)):
                pl.when(((tick & 1) == parity) & applies)(functools.partial(
                    fetch_unit, refs, tick >> 1, f["fetch_q"], f["fetch_h"], pattern))

        u, q, h = f["unit"], f["q"], f["h"]

        @pl.when(f["wait_q"] == 1)
        def _():
            _wait_filled(q_bf.at[q, pl.ds(h, HEADS // 2)], q_recv.at[h + q])

        pl.when(f["step"] == SCORES)(lambda: scores_step(u, q, h))
        pl.when(f["step"] == VALUES)(lambda: values_step(u - 1))

        @pl.when(f["step"] == BOTH)
        def _():
            _wait_filled(k_buf.at[u], k_sem.at[u])
            _wait_filled(v_buf.at[u - 1], v_sem.at[u - 1])
            weighted_values(u - 1)
            softmax_numerators(u, q, h)
            share(u - 1, acc_own, acc_in, acc_send, acc_recv)
            share(u, stat_own, stat_in, stat_send, stat_recv)

        @pl.when(f["job"] != 0)
        def _():
            for code, job in enumerate(jobs, start=1):
                pl.when(f["job"] == code)(functools.partial(job, f["job_arg"]))

    fetch_unit(k_refs, LAST, *UNITS[LAST])
    scores_step(LAST - 2, *UNITS[LAST - 2])
    values_step(LAST - 2)
    for b in range(N_KB):
        pltpu.make_async_copy(
            v_hbm.at[b, N_QB - 1, :, HEADS - 1], v_buf.at[LAST, pl.ds(b * BLK, BLK)],
            v_sem.at[LAST + 2 * b // N_KB]).start(priority=1)
    pl.when(is_0)(lambda: add_mid(N_QB - 1))
    scores_step(LAST - 1, *UNITS[LAST - 1])
    pl.when(is_0)(fetch_wo_last_head)
    values_step(LAST - 1)
    scores_step(LAST, *UNITS[LAST])
    for part in range(2):
        keys = _aligned(part, N_KEYS // 2)
        _wait_filled(v_buf.at[LAST, keys], v_sem.at[LAST + part])
        acc = _dot(p_bf[LAST & 1, :, keys], v_buf[LAST, keys].astype(BF16))
        if part == 0:
            acc_half[...] = acc
        else:
            acc_own[LAST] = (acc_half[...] + acc).astype(BF16)
    share(LAST, acc_own, acc_in, last_send, acc_recv)

    @pl.when(is_2)
    def _():
        pl.loop(N_EARLY, HEADS - 1)(functools.partial(fetch_128_rows, wo_hbm, wo_f32))
        fetch_wo_last_head()

        @pl.loop(0, N_QB)
        def _(q):
            ctx_mid[_aligned(q, BLK)] = merge(FIRST_MID + N_MID * q, N_MID, axis=1)
            for c in range(2):
                wait_early(c, q)

        pl.loop(N_EARLY, HEADS - 1)(cast_wo)
        for c, cols in enumerate(halves):
            out_acc[:, cols] = out_early[c].astype(F32) + _dot(
                ctx_mid[...], wo_bf[N_EARLY * DH:DM - DH, cols])

    @pl.when(is_odd)
    def _():
        fetch_wo_last_head()
        pl.loop(1, N_QB)(add_mid)

    def wait_sent(src, send, dev):
        _remote(src, src, send, wo_recv.at[0], dev).wait_send()

    def wait_shared(i, first):
        wait_sent(acc_own.at[first:LAST], acc_send.at[i], peers[i])
        wait_sent(stat_own.at[first:N_UNITS], stat_send.at[i], peers[i])

    pl.when(is_0)(lambda: wait_shared(0, FIRST_MID))
    pl.when(jnp.logical_not(is_0))(lambda: wait_shared(0, 0))
    for i in range(1, N_DEV - 1):
        wait_shared(i, FIRST_MID)

    @pl.when(is_0)
    def _():
        for i, dev in enumerate((1, 3)):
            wait_sent(out_early, job_send.at[i], dev)
            wait_sent(wo_mid, job_send.at[2 + i], dev)

    @pl.when(is_2)
    def _():
        for i, dev in enumerate((1, 3)):
            wait_sent(x_bf, job_send.at[i], dev)

    @pl.when(is_odd)
    def _():
        for i, dev in enumerate(peers):
            wait_sent(q_bf.at[:, _aligned(half, HEADS // 2)], job_send.at[i], dev)
        wait_sent(out_early.at[half], job_send.at[3], 2)

    top = SQ - BLK
    for c, cols in enumerate(halves):
        _wait_filled(wo_f32.at[last_head, cols], wo_last_sem.at[c])
        if c == 0:
            ctx = merge(FIRST_OF_LAST_HEAD, N_QB - 1, axis=0)
        else:
            _wait_filled(stat_in.at[LAST], stat_recv.at[LAST])
        w = wo_f32[last_head, cols].astype(BF16)
        wo_bf[last_head, cols] = w
        out_ref[0, 0:top, cols] = (out_acc[0:top, cols] + _dot(ctx, w)).astype(out_ref.dtype)

    weights = merge_weights(LAST)
    last_terms[0] = weights[0] * acc_own[LAST].astype(F32)
    for c in range(1, N_DEV):
        last_terms[c] = jnp.broadcast_to(weights[c], (BLK, DH))
    _wait_filled(acc_in.at[LAST], acc_recv.at[LAST])
    ctx = sum((last_terms[c + 1] * acc_in[LAST, c].astype(F32) for c in range(N_DEV - 1)),
              last_terms[0]).astype(BF16)
    out_ref[0, top:] = (out_acc[top:] + _dot(ctx, wo_bf[last_head])).astype(out_ref.dtype)

    for i, dev in enumerate(peers):
        wait_sent(acc_own.at[LAST], last_send.at[i], dev)


def pallas_dist_sparse_attn_strided_kvseq_b1_sq256_skv4096_hq8_dh128_kernel(
    x: jax.Array,
    Wq: jax.Array,
    K_ext: jax.Array,
    V_ext: jax.Array,
    Wo: jax.Array,
):
    kv_shape = (N_KB, N_QB, BLK, HEADS, DH)
    vmem, dma = pltpu.VMEM, pltpu.SemaphoreType.DMA
    return pl.pallas_call(
        _body,
        out_shape=jax.ShapeDtypeStruct((1, SQ, DM), BF16),
        in_specs=[pl.BlockSpec(memory_space=pltpu.HBM)] * 5,
        out_specs=pl.BlockSpec(memory_space=pltpu.VMEM),
        scratch_shapes=[
            vmem((N_UNITS, N_KEYS, DH), F32),
            vmem((N_UNITS, N_KEYS, DH), F32),
            vmem((SQ, DM), F32),
            vmem((DM, HALF), F32),
            vmem((DM, DM), F32),
            vmem((N_QB, BLK, DM), BF16),
            vmem((DM, HALF), BF16),
            vmem((DM, DM), BF16),
            vmem((N_QB, HEADS, BLK, DH), BF16),
            vmem((2, BLK, N_KEYS), BF16),
            vmem((N_UNITS, BLK, DH), BF16),
            vmem((N_UNITS, N_DEV - 1, BLK, DH), BF16),
            vmem((N_UNITS, 2, DH), F32),
            vmem((N_UNITS, N_DEV - 1, 2, DH), F32),
            vmem((BLK, N_EARLY * DH), BF16),
            vmem((SQ, N_MID * DH), BF16),
            vmem((2, SQ, HALF), BF16),
            vmem((SQ, DM), F32),
            vmem((BLK, DH), F32),
            vmem((N_DEV, BLK, DH), F32),
            pltpu.SMEM((N_TICKS,), jnp.int32),
            dma((N_UNITS,)),
            dma((N_UNITS + 1,)),
            dma((HEADS - 1,)),
            dma((2,)),
            dma((N_QB,)),
            dma((1,)),
            dma((2 * N_QB,)),
            dma((N_UNITS,)),
            dma((N_UNITS,)),
            dma((2 * N_QB,)),
            dma((N_DEV - 1,)),
            dma((N_DEV - 1,)),
            dma((N_DEV - 1,)),
            dma((N_DEV,)),
        ],
        compiler_params=pltpu.CompilerParams(
            collective_id=0,
            vmem_limit_bytes=64 * 1024 * 1024,
            disable_bounds_checks=True,
            disable_semaphore_checks=True,
        ),
    )(x.reshape(SQ, DM), Wq, K_ext.reshape(kv_shape), V_ext.reshape(kv_shape), Wo)
```
